```python
import numpy as np

kernel_name = "dist_argmax_global_i_m4096_n1024"

def setup_inputs():
    return {"x": np.random.randn(16384, 1024).astype(np.float32)}

def reference(x: np.ndarray) -> np.ndarray:
    idx = np.argmax(x, axis=0).astype(np.float32)
    val = np.max(x, axis=0)
    return np.stack([val, idx], axis=0)
```

```python
import jax
import jax.numpy as jnp
from jax import lax
from jax.experimental import pallas as pl
from jax.experimental.pallas import tpu as pltpu

N_DEV = 4
BLOCK_ROWS = 512
UNROLL = 8


def pallas_dist_argmax_global_i_m4096_n1024_kernel(
x: jax.Array,
):
    m_per, n = x.shape
    bm = BLOCK_ROWS
    assert m_per % bm == 0 and bm % 8 == 0
    n_steps = m_per // bm
    groups = bm // 8

    def body(x_ref, out_ref, acc_val, acc_idx, comm_ref, send_sems, recv_sems):
        step = pl.program_id(0)
        my = lax.axis_index("i")

        @pl.when(step == 0)
        def _init():
            barrier_sem = pltpu.get_barrier_semaphore()
            for k in range(1, N_DEV):
                pl.semaphore_signal(
                    barrier_sem, inc=1,
                    device_id=((my + k) % N_DEV,),
                    device_id_type=pl.DeviceIdType.MESH,
                )
            acc_val[...] = jnp.full(acc_val.shape, -jnp.inf, jnp.float32)
            acc_idx[...] = jnp.zeros(acc_idx.shape, jnp.int32)

        base = step * groups

        def loop(g, carry):
            v, i = carry
            xv = x_ref[pl.ds(pl.multiple_of(g * 8, 8), 8), :]
            m = xv > v
            v = jnp.where(m, xv, v)
            i = jnp.where(m, base + g, i)
            return v, i

        v, i = lax.fori_loop(0, groups, loop, (acc_val[...], acc_idx[...]),
                             unroll=UNROLL)
        acc_val[...] = v
        acc_idx[...] = i

        @pl.when(step == n_steps - 1)
        def _finish():
            sub = lax.broadcasted_iota(jnp.int32, (8, n), 0)
            rows = i * 8 + sub + my * m_per
            cmax = jnp.max(v, axis=0, keepdims=True)
            big = jnp.int32(2**30)
            cidx = jnp.min(jnp.where(v == cmax, rows, big), axis=0, keepdims=True)
            comm_ref[my, 0:1, :] = cmax
            comm_ref[my, 1:2, :] = cidx.astype(jnp.float32)

            barrier_sem = pltpu.get_barrier_semaphore()
            pl.semaphore_wait(barrier_sem, N_DEV - 1)

            copies = []
            for k in range(1, N_DEV):
                peer = (my + k) % N_DEV
                cp = pltpu.make_async_remote_copy(
                    src_ref=comm_ref.at[my],
                    dst_ref=comm_ref.at[my],
                    send_sem=send_sems.at[k - 1],
                    recv_sem=recv_sems.at[k - 1],
                    device_id=(peer,),
                    device_id_type=pl.DeviceIdType.MESH,
                )
                cp.start()
                copies.append(cp)
            for k in range(1, N_DEV):
                src = (my - k) % N_DEV
                rc = pltpu.make_async_remote_copy(
                    src_ref=comm_ref.at[src],
                    dst_ref=comm_ref.at[src],
                    send_sem=send_sems.at[k - 1],
                    recv_sem=recv_sems.at[k - 1],
                    device_id=(src,),
                    device_id_type=pl.DeviceIdType.MESH,
                )
                rc.wait_recv()
            for cp in copies:
                cp.wait_send()

            vals = comm_ref[:, 0, :]
            idxs = comm_ref[:, 1, :]
            gmax = jnp.max(vals, axis=0, keepdims=True)
            gidx = jnp.min(jnp.where(vals == gmax, idxs, jnp.float32(2**30)),
                           axis=0, keepdims=True)
            out_ref[0:1, :] = gmax
            out_ref[1:2, :] = gidx

    return pl.pallas_call(
        body,
        grid=(n_steps,),
        out_shape=jax.ShapeDtypeStruct((2, n), jnp.float32),
        in_specs=[pl.BlockSpec((bm, n), lambda s: (s, 0))],
        out_specs=pl.BlockSpec((2, n), lambda s: (0, 0)),
        scratch_shapes=[
            pltpu.VMEM((8, n), jnp.float32),
            pltpu.VMEM((8, n), jnp.int32),
            pltpu.VMEM((N_DEV, 2, n), jnp.float32),
            pltpu.SemaphoreType.DMA((N_DEV - 1,)),
            pltpu.SemaphoreType.DMA((N_DEV - 1,)),
        ],
        compiler_params=pltpu.CompilerParams(
            collective_id=0,
            dimension_semantics=("arbitrary",),
        ),
    )(x)
```

```python
import jax
import jax.numpy as jnp
from jax import lax
from jax.experimental import pallas as pl
from jax.experimental.pallas import tpu as pltpu

N_DEV = 4
CHUNK_ROWS = 64
N_BUF = 8


def pallas_dist_argmax_global_i_m4096_n1024_kernel(
x: jax.Array,
):
    m_per, n = x.shape
    bm = CHUNK_ROWS
    nbuf = N_BUF
    assert m_per % bm == 0 and bm % 8 == 0
    n_chunks = m_per // bm
    groups = bm // 8

    def body(x_hbm, out_ref, buf, dsem, comm_ref, send_sems, recv_sems):
        my = lax.axis_index("i")

        barrier_sem = pltpu.get_barrier_semaphore()
        for k in range(1, N_DEV):
            pl.semaphore_signal(
                barrier_sem, inc=1,
                device_id=((my + k) % N_DEV,),
                device_id_type=pl.DeviceIdType.MESH,
            )

        def dma(c, slot):
            return pltpu.make_async_copy(
                x_hbm.at[pl.ds(pl.multiple_of(c * bm, bm), bm), :],
                buf.at[slot], dsem.at[slot])

        for c in range(min(nbuf, n_chunks)):
            dma(c, c).start()

        def chunk_body(c, carry):
            slot = c % nbuf
            dma(c, slot).wait()
            base = c * groups
            v, i = carry
            for g in range(groups):
                xv = buf[slot, pl.ds(g * 8, 8), :]
                m = jnp.logical_and(jnp.logical_not(xv <= v), v == v)
                v = jnp.where(m, xv, v)
                i = jnp.where(m, base + g, i)

            @pl.when(c + nbuf < n_chunks)
            def _():
                dma(c + nbuf, slot).start()

            return v, i

        v0 = jnp.full((8, n), -jnp.inf, jnp.float32)
        i0 = jnp.zeros((8, n), jnp.int32)
        v, i = lax.fori_loop(0, n_chunks, chunk_body, (v0, i0))

        def reduce_rows(vals, idxs, big):
            isnan = vals != vals
            nan_flag = jnp.max(jnp.where(isnan, 1.0, 0.0), axis=0,
                               keepdims=True)
            vmax = jnp.max(jnp.where(isnan, -jnp.inf, vals), axis=0,
                           keepdims=True)
            no_nan = jnp.broadcast_to(nan_flag, vals.shape) == 0.0
            best = jnp.logical_or(
                isnan, jnp.logical_and(vals == vmax, no_nan))
            imin = jnp.min(jnp.where(best, idxs, big), axis=0, keepdims=True)
            vmax = jnp.where(nan_flag > 0.0, jnp.float32(jnp.nan), vmax)
            return vmax, imin

        sub = lax.broadcasted_iota(jnp.int32, (8, n), 0)
        rows = i * 8 + sub + my * m_per
        cmax, cidx = reduce_rows(v, rows, jnp.int32(2**30))
        comm_ref[my, 0:1, :] = cmax
        comm_ref[my, 1:2, :] = cidx.astype(jnp.float32)

        pl.semaphore_wait(barrier_sem, N_DEV - 1)

        copies = []
        for k in range(1, N_DEV):
            peer = (my + k) % N_DEV
            cp = pltpu.make_async_remote_copy(
                src_ref=comm_ref.at[my],
                dst_ref=comm_ref.at[my],
                send_sem=send_sems.at[k - 1],
                recv_sem=recv_sems.at[k - 1],
                device_id=(peer,),
                device_id_type=pl.DeviceIdType.MESH,
            )
            cp.start()
            copies.append(cp)
        for k in range(1, N_DEV):
            src = (my - k) % N_DEV
            rc = pltpu.make_async_remote_copy(
                src_ref=comm_ref.at[src],
                dst_ref=comm_ref.at[src],
                send_sem=send_sems.at[k - 1],
                recv_sem=recv_sems.at[k - 1],
                device_id=(src,),
                device_id_type=pl.DeviceIdType.MESH,
            )
            rc.wait_recv()
        for cp in copies:
            cp.wait_send()

        vals = comm_ref[:, 0, :]
        idxs = comm_ref[:, 1, :]
        gmax, gidx = reduce_rows(vals, idxs, jnp.float32(2**30))
        out_ref[0:1, :] = gmax
        out_ref[1:2, :] = gidx

    return pl.pallas_call(
        body,
        out_shape=jax.ShapeDtypeStruct((2, n), jnp.float32),
        in_specs=[pl.BlockSpec(memory_space=pl.ANY)],
        out_specs=pl.BlockSpec(memory_space=pltpu.VMEM),
        scratch_shapes=[
            pltpu.VMEM((nbuf, bm, n), jnp.float32),
            pltpu.SemaphoreType.DMA((nbuf,)),
            pltpu.VMEM((N_DEV, 2, n), jnp.float32),
            pltpu.SemaphoreType.DMA((N_DEV - 1,)),
            pltpu.SemaphoreType.DMA((N_DEV - 1,)),
        ],
        compiler_params=pltpu.CompilerParams(collective_id=0),
    )(x)
```
